```python
import numpy as np

kernel_name = "dist_moe_cap_ep_outshard_n2048_d512_e8_h1024"

def setup_inputs():
    x = np.random.randn(2048, 512).astype(np.float32)
    router_W = np.random.randn(512, 32).astype(np.float32) * 0.1
    scores64 = x.astype(np.float64) @ router_W.astype(np.float64)
    route_idx = np.argsort(-scores64, axis=-1)[:, :1].astype(np.int32)
    expert_W = np.random.randn(32, 512, 1024).astype(np.float32) * 0.02
    return {"x": x, "router_W": router_W, "route_idx": route_idx, "expert_W": expert_W}

def reference(x, router_W, route_idx, expert_W):
    counts = np.zeros(32, dtype=np.int64)
    out = np.zeros((2048, 1024), dtype=np.float32)
    for i in range(2048):
        e = int(route_idx[i, 0])
        if counts[e] < 51:
            out[i] = x[i] @ expert_W[e]
            counts[e] += 1
    return out
```

```python
import jax
import jax.numpy as jnp
from jax import lax
from jax.experimental import pallas as pl
from jax.experimental.pallas import tpu as pltpu

N_TOK = 2048
D = 512
H = 1024
E = 32
E_LOC = 8
CAP = 51
NDEV = 4
ROWS = N_TOK // NDEV
SLOT = 64
MROWS = 56
NB = N_TOK // 128


def _kernel(idx_ref, x_hbm, w_hbm, out_hbm,
            wbuf, xg, res, zbuf, tab_v, keep_v, tab_s, keep_s,
            wsem, gsem, tsem, send_sem, recv_sem):
    me = lax.axis_index("i")
    f32 = jnp.float32
    bf16 = jnp.bfloat16
    i32 = jnp.int32

    def w_copy(e):
        return pltpu.make_async_copy(w_hbm.at[e], wbuf.at[e], wsem.at[e])

    for e in range(E_LOC):
        w_copy(e).start()

    barrier = pltpu.get_barrier_semaphore()
    for k in range(1, NDEV):
        pl.semaphore_signal(barrier, inc=1, device_id=((me + k) % NDEV,),
                            device_id_type=pl.DeviceIdType.MESH)

    zbuf[...] = jnp.zeros_like(zbuf)

    idx = idx_ref[...]
    e_iota = lax.broadcasted_iota(i32, (E, NB, 128), 0)
    oh = (idx[None] == e_iota).astype(f32).reshape(E * NB, 128)
    r = lax.broadcasted_iota(i32, (128, 256), 0)
    c = lax.broadcasted_iota(i32, (128, 256), 1)
    rhs = jnp.where((r < c) | (c >= 128), 1.0, 0.0).astype(bf16)
    t = jnp.dot(oh.astype(bf16), rhs, preferred_element_type=f32)
    within = t[:, :128]
    tot = t[:, 128:]
    R = lax.broadcasted_iota(i32, (E * NB, E * NB), 0)
    C = lax.broadcasted_iota(i32, (E * NB, E * NB), 1)
    lblk = jnp.where(((R // NB) == (C // NB)) & (C < R), 1.0, 0.0).astype(bf16)
    cross = jnp.dot(lblk, tot.astype(bf16), preferred_element_type=f32)
    prefix = within + cross
    pos = (oh * prefix).reshape(E, NB, 128).sum(axis=0).astype(i32)
    keep = pos < CAP
    local = (idx >> 3) == me
    slot = jnp.where(local & keep, (idx & 7) * SLOT + pos, -1)
    keep_v[...] = keep.astype(i32)

    nslot = E_LOC * SLOT
    s_iota = lax.broadcasted_iota(i32, (nslot, 128), 0)
    lane = lax.broadcasted_iota(i32, (1, 128), 1)
    acc = jnp.zeros((nslot, 128), i32)
    for b in range(NB):
        m = slot[b:b + 1, :] == s_iota
        acc = acc + jnp.where(m, lane + (b * 128 + 1), 0)
    hilo = jnp.concatenate([(acc >> 6).astype(f32), (acc & 63).astype(f32)],
                           axis=0).astype(bf16)
    ones = jnp.ones((8, 128), bf16)
    red = lax.dot_general(ones, hilo, (((1,), (1,)), ((), ())),
                          preferred_element_type=f32)
    tab = red[:, :nslot] * 64.0 + red[:, nslot:] - 1.0
    tab_v[...] = tab.astype(i32)

    c1 = pltpu.make_async_copy(tab_v.at[pl.ds(0, 1)], tab_s, tsem.at[0])
    c2 = pltpu.make_async_copy(keep_v, keep_s, tsem.at[1])
    c1.start()
    c2.start()
    c1.wait()
    c2.wait()

    for e in range(E_LOC):
        def gbody(s, carry, e=e):
            tok = jnp.maximum(tab_s[0, e * SLOT + s], 0)
            pltpu.make_async_copy(x_hbm.at[pl.ds(tok, 1)],
                                  xg.at[e, pl.ds(s, 1)], gsem.at[e]).start()
            return carry
        lax.fori_loop(0, CAP, gbody, 0)

    def zbody(rr, carry):
        k = keep_s[me * 4 + (rr >> 7), rr & 127]

        @pl.when(k == 0)
        def _():
            pltpu.make_async_copy(zbuf.at[pl.ds(0, 1)],
                                  out_hbm.at[pl.ds(rr, 1)], recv_sem).start()
        return carry
    lax.fori_loop(0, ROWS, zbody, 0)

    pl.semaphore_wait(barrier, NDEV - 1)

    nsent = jnp.int32(0)
    for e in range(E_LOC):
        n8 = (CAP // 8) * 8
        pltpu.make_async_copy(xg.at[e, pl.ds(0, n8)], xg.at[e, pl.ds(0, n8)],
                              gsem.at[e]).wait()
        for s in range(n8, CAP):
            pltpu.make_async_copy(xg.at[e, pl.ds(s, 1)], xg.at[e, pl.ds(s, 1)],
                                  gsem.at[e]).wait()
        w_copy(e).wait()
        res[e] = jnp.dot(xg[e].astype(bf16), wbuf[e].astype(bf16),
                         preferred_element_type=f32)

        def sbody(s, n, e=e):
            tok = tab_s[0, e * SLOT + s]

            @pl.when(tok >= 0)
            def _():
                pltpu.make_async_remote_copy(
                    res.at[e, pl.ds(s, 1)],
                    out_hbm.at[pl.ds(tok & (ROWS - 1), 1)],
                    send_sem, recv_sem,
                    device_id=(tok >> 9,),
                    device_id_type=pl.DeviceIdType.MESH).start()
            return n + (tok >= 0).astype(i32)
        nsent = lax.fori_loop(0, CAP, sbody, nsent)

    def wbody(j, carry):
        pltpu.make_async_remote_copy(
            res.at[0, pl.ds(0, 1)], out_hbm.at[pl.ds(0, 1)],
            send_sem, recv_sem, device_id=(me,),
            device_id_type=pl.DeviceIdType.MESH).wait_send()
        return carry
    lax.fori_loop(0, nsent, wbody, 0)
    pltpu.make_async_copy(out_hbm, out_hbm, recv_sem).wait()


def pallas_dist_moe_cap_ep_outshard_n2048_d512_e8_h1024_kernel(
    x: jax.Array,
    router_W: jax.Array,
    route_idx: jax.Array,
    expert_W: jax.Array,
):
    del router_W
    idx2d = route_idx.astype(jnp.int32).reshape(NB, 128)
    return pl.pallas_call(
        _kernel,
        out_shape=jax.ShapeDtypeStruct((ROWS, H), jnp.float32),
        in_specs=[
            pl.BlockSpec(memory_space=pltpu.VMEM),
            pl.BlockSpec(memory_space=pl.ANY),
            pl.BlockSpec(memory_space=pl.ANY),
        ],
        out_specs=pl.BlockSpec(memory_space=pl.ANY),
        scratch_shapes=[
            pltpu.VMEM((E_LOC, D, H), jnp.float32),
            pltpu.VMEM((E_LOC, MROWS, D), jnp.float32),
            pltpu.VMEM((E_LOC, MROWS, H), jnp.float32),
            pltpu.VMEM((8, H), jnp.float32),
            pltpu.VMEM((8, E_LOC * SLOT), jnp.int32),
            pltpu.VMEM((NB, 128), jnp.int32),
            pltpu.SMEM((1, E_LOC * SLOT), jnp.int32),
            pltpu.SMEM((NB, 128), jnp.int32),
            pltpu.SemaphoreType.DMA((E_LOC,)),
            pltpu.SemaphoreType.DMA((E_LOC,)),
            pltpu.SemaphoreType.DMA((2,)),
            pltpu.SemaphoreType.DMA,
            pltpu.SemaphoreType.DMA,
        ],
        compiler_params=pltpu.CompilerParams(
            collective_id=0,
            vmem_limit_bytes=64 * 1024 * 1024,
        ),
    )(idx2d, x, expert_W)
```

```python
import jax
import jax.numpy as jnp
from jax import lax
from jax.experimental import pallas as pl
from jax.experimental.pallas import tpu as pltpu

N_TOK = 2048
D = 512
H = 1024
E = 32
E_LOC = 8
CAP = 51
NDEV = 4
ROWS = N_TOK // NDEV
SLOT = 64
MROWS = 56
NB = N_TOK // 128
SCOPES = False
import contextlib
def scope(name):
    return jax.named_scope(name) if SCOPES else contextlib.nullcontext()


def _kernel(idx_ref, x_hbm, w_hbm, out_ref,
            wbuf, xg, res, pad_src, pad_dst, tab_v, tab_s,
            wsem, gsem, tsem, send_sem, recv_sem):
    me = lax.axis_index("i")
    f32 = jnp.float32
    bf16 = jnp.bfloat16
    i32 = jnp.int32

    def w_copy(e):
        return pltpu.make_async_copy(w_hbm.at[e], wbuf.at[e], wsem.at[e])

    for e in range(E_LOC):
        w_copy(e).start(priority=1)

    with scope("zero"):
        out_ref[...] = jnp.zeros_like(out_ref)
        pad_src[...] = jnp.zeros_like(pad_src)

    barrier = pltpu.get_barrier_semaphore()
    for k in range(1, NDEV):
        pl.semaphore_signal(barrier, inc=1, device_id=((me + k) % NDEV,),
                            device_id_type=pl.DeviceIdType.MESH)

    with scope("route"):
        idx = idx_ref[...]
        e_iota = lax.broadcasted_iota(i32, (E, NB, 128), 0)
        oh = (idx[None] == e_iota).astype(f32).reshape(E * NB, 128)
        r = lax.broadcasted_iota(i32, (128, 256), 0)
        c = lax.broadcasted_iota(i32, (128, 256), 1)
        rhs = jnp.where((r < c) | (c >= 128), 1.0, 0.0).astype(bf16)
        t = jnp.dot(oh.astype(bf16), rhs, preferred_element_type=f32)
        within = t[:, :128]
        tot = t[:, 128:]
        R = lax.broadcasted_iota(i32, (E * NB, E * NB), 0)
        C = lax.broadcasted_iota(i32, (E * NB, E * NB), 1)
        lblk = jnp.where(((R // NB) == (C // NB)) & (C < R), 1.0, 0.0).astype(bf16)
        cross = jnp.dot(lblk, tot.astype(bf16), preferred_element_type=f32)
        prefix = within + cross
        pos = (oh * prefix).reshape(E, NB, 128).sum(axis=0).astype(i32)
        keep = pos < CAP
        local = (idx >> 3) == me
        slot = jnp.where(local & keep, (idx & 7) * SLOT + pos, -1)

        blk = lax.broadcasted_iota(i32, (NB, 128), 0)
        dropf = jnp.where(((blk >> 2) == me) & jnp.logical_not(keep), 1.0, 0.0)
        dcol = jnp.dot(jnp.ones((8, NB), bf16), dropf.astype(bf16),
                       preferred_element_type=f32)
        nslot = E_LOC * SLOT
        ndrop = jnp.dot(dcol.astype(bf16), jnp.ones((128, nslot), bf16),
                        preferred_element_type=f32)

        s_iota = lax.broadcasted_iota(i32, (nslot, 128), 0)
        lane = lax.broadcasted_iota(i32, (1, 128), 1)
        acc = jnp.zeros((nslot, 128), i32)
        for b in range(NB):
            m = slot[b:b + 1, :] == s_iota
            acc = acc + jnp.where(m, lane + (b * 128 + 1), 0)
        hilo = jnp.concatenate([(acc >> 6).astype(f32), (acc & 63).astype(f32)],
                               axis=0).astype(bf16)
        red = lax.dot_general(jnp.ones((8, 128), bf16), hilo,
                              (((1,), (1,)), ((), ())),
                              preferred_element_type=f32)
        tab = red[:, :nslot] * 64.0 + red[:, nslot:] - 1.0
        sl = lax.broadcasted_iota(i32, (8, nslot), 1)
        tab = jnp.where(sl == SLOT - 1, ndrop, tab)
        tab_v[...] = tab.astype(i32)

    with scope("tabdma"):
        c1 = pltpu.make_async_copy(tab_v.at[pl.ds(0, 1)], tab_s, tsem)
        c1.start()
        c1.wait()

    def gather(e):
        for s in range(CAP):
            tok = jnp.maximum(tab_s[0, e * SLOT + s], 0)
            pltpu.make_async_copy(x_hbm.at[pl.ds(tok, 1)],
                                  xg.at[e, pl.ds(s, 1)], gsem.at[e]).start()

    with scope("gather01"):
        gather(0)
        gather(1)

    with scope("topup"):
        nd = tab_s[0, SLOT - 1]
        for bit in range(6):
            sz = 8 << bit

            @pl.when(((nd >> (3 + bit)) & 1) == 1)
            def _(sz=sz):
                pltpu.make_async_copy(pad_src.at[pl.ds(0, sz)],
                                      pad_dst.at[pl.ds(sz, sz)], recv_sem).start()

        @pl.when(nd >= ROWS)
        def _():
            pltpu.make_async_copy(pad_src, pad_dst.at[pl.ds(ROWS, ROWS)],
                                  recv_sem).start()
        for j in range(7):
            @pl.when((nd & 7) > j)
            def _(j=j):
                pltpu.make_async_copy(pad_src.at[pl.ds(j, 1)],
                                      pad_dst.at[pl.ds(j, 1)], recv_sem).start()

    with scope("barwait"):
        pl.semaphore_wait(barrier, NDEV - 1)

    nsent = jnp.int32(0)
    for e in range(E_LOC):
        with scope(f"wait{e}"):
            n8 = (CAP // 8) * 8
            pltpu.make_async_copy(xg.at[e, pl.ds(0, n8)], xg.at[e, pl.ds(0, n8)],
                                  gsem.at[e]).wait()
            for s in range(n8, CAP):
                pltpu.make_async_copy(xg.at[e, pl.ds(s, 1)], xg.at[e, pl.ds(s, 1)],
                                      gsem.at[e]).wait()
            w_copy(e).wait()
        with scope(f"mm{e}"):
            res[e] = jnp.dot(xg[e].astype(bf16), wbuf[e].astype(bf16),
                             preferred_element_type=f32)
        with scope(f"send{e}"):
            for s in range(CAP):
                tok = tab_s[0, e * SLOT + s]

                @pl.when(tok >= 0)
                def _(tok=tok, s=s, e=e):
                    pltpu.make_async_remote_copy(
                        res.at[e, pl.ds(s, 1)],
                        out_ref.at[pl.ds(tok & (ROWS - 1), 1)],
                        send_sem, recv_sem,
                        device_id=(tok >> 9,),
                        device_id_type=pl.DeviceIdType.MESH).start()
                nsent = nsent + (tok >= 0).astype(i32)
        if e + 2 < E_LOC:
            with scope(f"gather{e+2}"):
                gather(e + 2)

    with scope("drain_send"):
        def w8(j, carry):
            pltpu.make_async_remote_copy(
                res.at[0, pl.ds(0, 8)], out_ref.at[pl.ds(0, 8)],
                send_sem, recv_sem, device_id=(me,),
                device_id_type=pl.DeviceIdType.MESH).wait_send()
            return carry
        lax.fori_loop(0, nsent >> 3, w8, 0)

        def w1(j, carry):
            pltpu.make_async_remote_copy(
                res.at[0, pl.ds(0, 1)], out_ref.at[pl.ds(0, 1)],
                send_sem, recv_sem, device_id=(me,),
                device_id_type=pl.DeviceIdType.MESH).wait_send()
            return carry
        lax.fori_loop(0, nsent & 7, w1, 0)
    with scope("drain_recv"):
        pltpu.make_async_copy(out_ref, out_ref, recv_sem).wait()


def pallas_dist_moe_cap_ep_outshard_n2048_d512_e8_h1024_kernel(
    x: jax.Array,
    router_W: jax.Array,
    route_idx: jax.Array,
    expert_W: jax.Array,
):
    del router_W
    idx2d = route_idx.astype(jnp.int32).reshape(NB, 128)
    return pl.pallas_call(
        _kernel,
        out_shape=jax.ShapeDtypeStruct((ROWS, H), jnp.float32),
        in_specs=[
            pl.BlockSpec(memory_space=pltpu.VMEM),
            pl.BlockSpec(memory_space=pl.ANY),
            pl.BlockSpec(memory_space=pl.ANY),
        ],
        out_specs=pl.BlockSpec(memory_space=pltpu.VMEM),
        scratch_shapes=[
            pltpu.VMEM((E_LOC, D, H), jnp.float32),
            pltpu.VMEM((E_LOC, MROWS, D), jnp.float32),
            pltpu.VMEM((E_LOC, MROWS, H), jnp.float32),
            pltpu.VMEM((ROWS, H), jnp.float32),
            pltpu.VMEM((2 * ROWS, H), jnp.float32),
            pltpu.VMEM((8, E_LOC * SLOT), jnp.int32),
            pltpu.SMEM((1, E_LOC * SLOT), jnp.int32),
            pltpu.SemaphoreType.DMA((E_LOC,)),
            pltpu.SemaphoreType.DMA((E_LOC,)),
            pltpu.SemaphoreType.DMA,
            pltpu.SemaphoreType.DMA,
            pltpu.SemaphoreType.DMA,
        ],
        compiler_params=pltpu.CompilerParams(
            collective_id=0,
            vmem_limit_bytes=64 * 1024 * 1024,
            disable_bounds_checks=True,
        ),
    )(idx2d, x, expert_W)
```

```python
import contextlib

import jax
import jax.numpy as jnp
from jax import lax
from jax.experimental import pallas as pl
from jax.experimental.pallas import tpu as pltpu

N_TOK = 2048
D = 512
H = 1024
E = 32
E_LOC = 8
CAP = 51
NDEV = 4
ROWS = N_TOK // NDEV
SLOT = 64
NSLOT = E_LOC * SLOT
MROWS = 56
HW = H // 2
QW = H // 4
NB = N_TOK // 128
NSEND = E_LOC * CAP
RECV_ROWS = ROWS + NSEND
KSPLIT = 4
SCOPES = False


def scope(name):
    return jax.named_scope(name) if SCOPES else contextlib.nullcontext()


def _kernel(idx_hbm, x_hbm, w_hbm, out_ref,
            idx_v, wbuf, xg, res, stage, pad_src, pad_dst, tab_v, tab_s,
            isem, wsem, gsem, tsem, send_sem, recv_sem):
    me = lax.axis_index("i")
    f32 = jnp.float32
    bf16 = jnp.bfloat16
    i32 = jnp.int32
    u32 = jnp.uint32
    last = E_LOC - 1
    kc = D // KSPLIT

    def w_copy(e):
        return pltpu.make_async_copy(w_hbm.at[e], wbuf.at[e], wsem.at[e])

    def w_last_copy(k):
        if k == 0:
            return pltpu.make_async_copy(w_hbm.at[last, :, pl.ds(0, HW)],
                                         wbuf.at[last, :, pl.ds(0, HW)],
                                         wsem.at[last])
        return pltpu.make_async_copy(
            w_hbm.at[last, pl.ds((k - 1) * kc, kc), pl.ds(HW, HW)],
            wbuf.at[last, pl.ds((k - 1) * kc, kc), pl.ds(HW, HW)],
            wsem.at[last + k])

    def pack(y):
        yb = lax.bitcast_convert_type(y.astype(bf16).astype(f32), u32)
        return (yb[:, :QW] >> 16) | (yb[:, QW:] & jnp.uint32(0xFFFF0000))

    def send_rows(e, c0, cw):
        for s in range(CAP):
            code = tab_s[1, e * SLOT + s]
            pltpu.make_async_remote_copy(
                res.at[e, pl.ds(s, 1), pl.ds(c0, cw)],
                stage.at[pl.ds(code & (2 * ROWS - 1), 1), pl.ds(c0, cw)],
                send_sem, recv_sem,
                device_id=(code >> 10,),
                device_id_type=pl.DeviceIdType.MESH).start()

    idx_copy = pltpu.make_async_copy(idx_hbm, idx_v, isem)
    idx_copy.start()
    for e in range(last):
        w_copy(e).start(priority=1)
    for k in range(KSPLIT + 1):
        w_last_copy(k).start(priority=1)

    with scope("zero"):
        stage[pl.ds(0, ROWS), :] = jnp.zeros((ROWS, HW), u32)
        pad_src[...] = jnp.zeros_like(pad_src)

    barrier = pltpu.get_barrier_semaphore()
    for k in range(1, NDEV):
        pl.semaphore_signal(barrier, inc=1, device_id=((me + k) % NDEV,),
                            device_id_type=pl.DeviceIdType.MESH)

    idx_copy.wait()
    with scope("route"):
        idx = idx_v[...]
        e_iota = lax.broadcasted_iota(i32, (E, NB, 128), 0)
        oh = (idx[None] == e_iota).astype(f32).reshape(E * NB, 128)
        r = lax.broadcasted_iota(i32, (128, 256), 0)
        c = lax.broadcasted_iota(i32, (128, 256), 1)
        rhs = jnp.where((r < c) | (c >= 128), 1.0, 0.0).astype(bf16)
        t = jnp.dot(oh.astype(bf16), rhs, preferred_element_type=f32)
        within = t[:, :128]
        tot = t[:, 128:]
        R = lax.broadcasted_iota(i32, (E * NB, E * NB), 0)
        C = lax.broadcasted_iota(i32, (E * NB, E * NB), 1)
        lblk = jnp.where(((R // NB) == (C // NB)) & (C < R), 1.0, 0.0).astype(bf16)
        cross = jnp.dot(lblk, tot.astype(bf16), preferred_element_type=f32)
        prefix = within + cross
        pos = (oh * prefix).reshape(E, NB, 128).sum(axis=0).astype(i32)
        keep = pos < CAP
        mine = ((idx >> 3) == me) & keep
        slot = jnp.where(mine, (idx & 7) * SLOT + pos, -1)

        blk = lax.broadcasted_iota(i32, (NB, 128), 0)
        padf = (jnp.where(((blk >> 2) == me) & jnp.logical_not(keep), 1.0, 0.0)
                + jnp.where(mine, 1.0, 0.0))
        pcol = jnp.dot(jnp.ones((8, NB), bf16), padf.astype(bf16),
                       preferred_element_type=f32)
        npad = jnp.dot(pcol.astype(bf16), jnp.ones((128, NSLOT), bf16),
                       preferred_element_type=f32)

        s_iota = lax.broadcasted_iota(i32, (NSLOT, 128), 0)
        lane = lax.broadcasted_iota(i32, (1, 128), 1)
        acc = jnp.zeros((NSLOT, 128), i32)
        for b in range(NB):
            m = slot[b:b + 1, :] == s_iota
            acc = acc + jnp.where(m, lane + (b * 128 + 1), 0)
        hilo = jnp.concatenate([(acc >> 6).astype(f32), (acc & 63).astype(f32)],
                               axis=0).astype(bf16)
        red = lax.dot_general(jnp.ones((8, 128), bf16), hilo,
                              (((1,), (1,)), ((), ())),
                              preferred_element_type=f32)
        tok = (red[:, :NSLOT] * 64.0 + red[:, NSLOT:] - 1.0).astype(i32)
        sl = lax.broadcasted_iota(i32, (8, NSLOT), 1)
        sub = lax.broadcasted_iota(i32, (8, NSLOT), 0)
        valid = tok >= 0
        src_row = jnp.where(valid, tok, 0)
        dst_code = jnp.where(valid, ((tok >> 9) << 10) | (tok & (ROWS - 1)),
                             (me << 10) | (ROWS + sl))
        tab = jnp.where(sub == 0, src_row, dst_code)
        tab = jnp.where(sl == SLOT - 1, npad.astype(i32), tab)
        tab_v[...] = tab

    with scope("tabdma"):
        c1 = pltpu.make_async_copy(tab_v.at[pl.ds(0, 1)], tab_s.at[pl.ds(0, 1)],
                                   tsem.at[0])
        c2 = pltpu.make_async_copy(tab_v.at[pl.ds(1, 1)], tab_s.at[pl.ds(1, 1)],
                                   tsem.at[1])
        c1.start()
        c2.start()
        c1.wait()
        c2.wait()

    def gather(e):
        for s in range(CAP):
            pltpu.make_async_copy(x_hbm.at[pl.ds(tab_s[0, e * SLOT + s], 1)],
                                  xg.at[e, pl.ds(s, 1)], gsem.at[e]).start()

    with scope("gather01"):
        gather(0)
        gather(1)

    with scope("topup"):
        nd = tab_s[0, SLOT - 1]
        for bit in range(7):
            sz = 8 << bit

            @pl.when(((nd >> (3 + bit)) & 1) == 1)
            def _(sz=sz):
                pltpu.make_async_copy(pad_src.at[pl.ds(0, sz)],
                                      pad_dst.at[pl.ds(sz, sz)], recv_sem).start()
        for j in range(7):
            @pl.when((nd & 7) > j)
            def _(j=j):
                pltpu.make_async_copy(pad_src.at[pl.ds(j, 1)],
                                      pad_dst.at[pl.ds(j, 1)], recv_sem).start()

    with scope("barwait"):
        pl.semaphore_wait(barrier, NDEV - 1)

    for e in range(E_LOC):
        with scope(f"wait{e}"):
            n8 = (CAP // 8) * 8
            pltpu.make_async_copy(xg.at[e, pl.ds(0, n8)], xg.at[e, pl.ds(0, n8)],
                                  gsem.at[e]).wait()
            for s in range(n8, CAP):
                pltpu.make_async_copy(xg.at[e, pl.ds(s, 1)], xg.at[e, pl.ds(s, 1)],
                                      gsem.at[e]).wait()
        if e < last:
            with scope(f"mm{e}"):
                w_copy(e).wait()
                y = jnp.dot(xg[e].astype(bf16), wbuf[e].astype(bf16),
                            preferred_element_type=f32)
                res[e, :, :QW] = pack(y[:, :HW])
                res[e, :, QW:] = pack(y[:, HW:])
            with scope(f"send{e}"):
                send_rows(e, 0, HW)
        else:
            with scope(f"mm{e}a"):
                w_last_copy(0).wait()
                y = jnp.dot(xg[e].astype(bf16), wbuf[e, :, :HW].astype(bf16),
                            preferred_element_type=f32)
                res[e, :, :QW] = pack(y)
            with scope(f"send{e}a"):
                send_rows(e, 0, QW)
            with scope(f"mm{e}b"):
                y = None
                for k in range(KSPLIT):
                    w_last_copy(k + 1).wait()
                    p = jnp.dot(xg[e, :, k * kc:(k + 1) * kc].astype(bf16),
                                wbuf[e, k * kc:(k + 1) * kc, HW:].astype(bf16),
                                preferred_element_type=f32)
                    y = p if y is None else y + p
                res[e, :, QW:] = pack(y)
            with scope(f"send{e}b"):
                send_rows(e, QW, QW)
        if e + 2 < E_LOC:
            with scope(f"gather{e+2}"):
                gather(e + 2)

    with scope("drain_send"):
        pltpu.make_async_remote_copy(
            stage.at[pl.ds(0, NSEND)], stage.at[pl.ds(0, NSEND)],
            send_sem, recv_sem, device_id=(me,),
            device_id_type=pl.DeviceIdType.MESH).wait_send()
    with scope("drain_recv"):
        pltpu.make_async_copy(stage.at[pl.ds(0, RECV_ROWS)],
                              stage.at[pl.ds(0, RECV_ROWS)], recv_sem).wait()
    with scope("unpack"):
        w = stage[pl.ds(0, ROWS), :]
        lo = lax.bitcast_convert_type(w << 16, f32)
        hi = lax.bitcast_convert_type(w & jnp.uint32(0xFFFF0000), f32)
        out_ref[:, 0 * QW:1 * QW] = lo[:, :QW]
        out_ref[:, 1 * QW:2 * QW] = hi[:, :QW]
        out_ref[:, 2 * QW:3 * QW] = lo[:, QW:]
        out_ref[:, 3 * QW:4 * QW] = hi[:, QW:]


def pallas_dist_moe_cap_ep_outshard_n2048_d512_e8_h1024_kernel(
    x: jax.Array,
    router_W: jax.Array,
    route_idx: jax.Array,
    expert_W: jax.Array,
):
    del router_W
    idx2d = route_idx.astype(jnp.int32).reshape(NB, 128)
    return pl.pallas_call(
        _kernel,
        out_shape=jax.ShapeDtypeStruct((ROWS, H), jnp.float32),
        in_specs=[
            pl.BlockSpec(memory_space=pl.ANY),
            pl.BlockSpec(memory_space=pl.ANY),
            pl.BlockSpec(memory_space=pl.ANY),
        ],
        out_specs=pl.BlockSpec(memory_space=pltpu.VMEM),
        scratch_shapes=[
            pltpu.VMEM((NB, 128), jnp.int32),
            pltpu.VMEM((E_LOC, D, H), jnp.float32),
            pltpu.VMEM((E_LOC, MROWS, D), jnp.float32),
            pltpu.VMEM((E_LOC, MROWS, HW), jnp.uint32),
            pltpu.VMEM((2 * ROWS, HW), jnp.uint32),
            pltpu.VMEM((ROWS, HW), jnp.uint32),
            pltpu.VMEM((2 * ROWS, HW), jnp.uint32),
            pltpu.VMEM((8, NSLOT), jnp.int32),
            pltpu.SMEM((2, NSLOT), jnp.int32),
            pltpu.SemaphoreType.DMA,
            pltpu.SemaphoreType.DMA((E_LOC + KSPLIT,)),
            pltpu.SemaphoreType.DMA((E_LOC,)),
            pltpu.SemaphoreType.DMA((2,)),
            pltpu.SemaphoreType.DMA,
            pltpu.SemaphoreType.DMA,
        ],
        compiler_params=pltpu.CompilerParams(
            collective_id=0,
            vmem_limit_bytes=64 * 1024 * 1024,
            disable_bounds_checks=True,
        ),
    )(idx2d, x, expert_W)
```

```python
import jax
import jax.numpy as jnp
from jax import lax
from jax.experimental import pallas as pl
from jax.experimental.pallas import tpu as pltpu

N_TOK = 2048
D = 512
H = 1024
E = 32
E_LOC = 8
CAP = 51
NDEV = 4
ROWS = N_TOK // NDEV
SLOT = 64
NSLOT = E_LOC * SLOT
MROWS = 56
HW = H // 2
QW = H // 4
NB = N_TOK // 128
NSEND = E_LOC * CAP
RECV_ROWS = ROWS + NSEND
KSPLIT = 4


def _kernel(idx_hbm, x_hbm, w_hbm, out_ref,
            idx_v, wbuf, xg, res, stage, pad_src, pad_dst, tab_v, tab_s,
            isem, wsem, gsem, tsem, send_sem, recv_sem):
    me = lax.axis_index("i")
    f32 = jnp.float32
    bf16 = jnp.bfloat16
    i32 = jnp.int32
    u32 = jnp.uint32
    last = E_LOC - 1
    kc = D // KSPLIT

    def w_copy(e):
        return pltpu.make_async_copy(w_hbm.at[e], wbuf.at[e], wsem.at[e])

    def w_last_copy(k):
        if k == 0:
            return pltpu.make_async_copy(w_hbm.at[last, :, pl.ds(0, HW)],
                                         wbuf.at[last, :, pl.ds(0, HW)],
                                         wsem.at[last])
        return pltpu.make_async_copy(
            w_hbm.at[last, pl.ds((k - 1) * kc, kc), pl.ds(HW, HW)],
            wbuf.at[last, pl.ds((k - 1) * kc, kc), pl.ds(HW, HW)],
            wsem.at[last + k])

    def pack(y):
        yb = lax.bitcast_convert_type(y.astype(bf16).astype(f32), u32)
        return (yb[:, :QW] >> 16) | (yb[:, QW:] & jnp.uint32(0xFFFF0000))

    def gather(e):
        for s in range(CAP):
            pltpu.make_async_copy(x_hbm.at[pl.ds(tab_s[0, e * SLOT + s], 1)],
                                  xg.at[e, pl.ds(s, 1)], gsem.at[e]).start()

    def send_rows(e, c0, cw):
        for s in range(CAP):
            code = tab_s[1, e * SLOT + s]
            pltpu.make_async_remote_copy(
                res.at[e, pl.ds(s, 1), pl.ds(c0, cw)],
                stage.at[pl.ds(code & (2 * ROWS - 1), 1), pl.ds(c0, cw)],
                send_sem, recv_sem,
                device_id=(code >> 10,),
                device_id_type=pl.DeviceIdType.MESH).start()

    idx_copy = pltpu.make_async_copy(idx_hbm, idx_v, isem)
    idx_copy.start()
    for e in range(last):
        w_copy(e).start(priority=1)
    for k in range(KSPLIT + 1):
        w_last_copy(k).start(priority=1)

    stage[pl.ds(0, ROWS), :] = jnp.zeros((ROWS, HW), u32)
    pad_src[...] = jnp.zeros_like(pad_src)

    barrier = pltpu.get_barrier_semaphore()
    for k in range(1, NDEV):
        pl.semaphore_signal(barrier, inc=1, device_id=((me + k) % NDEV,),
                            device_id_type=pl.DeviceIdType.MESH)

    idx_copy.wait()
    idx = idx_v[...]
    e_iota = lax.broadcasted_iota(i32, (E, NB, 128), 0)
    oh = (idx[None] == e_iota).astype(f32).reshape(E * NB, 128)
    r = lax.broadcasted_iota(i32, (128, 256), 0)
    c = lax.broadcasted_iota(i32, (128, 256), 1)
    rhs = jnp.where((r < c) | (c >= 128), 1.0, 0.0).astype(bf16)
    t = jnp.dot(oh.astype(bf16), rhs, preferred_element_type=f32)
    within = t[:, :128]
    tot = t[:, 128:]
    R = lax.broadcasted_iota(i32, (E * NB, E * NB), 0)
    C = lax.broadcasted_iota(i32, (E * NB, E * NB), 1)
    lblk = jnp.where(((R // NB) == (C // NB)) & (C < R), 1.0, 0.0).astype(bf16)
    cross = jnp.dot(lblk, tot.astype(bf16), preferred_element_type=f32)
    prefix = within + cross
    pos = (oh * prefix).reshape(E, NB, 128).sum(axis=0).astype(i32)
    keep = pos < CAP
    mine = ((idx >> 3) == me) & keep
    slot = jnp.where(mine, (idx & 7) * SLOT + pos, -1)

    blk = lax.broadcasted_iota(i32, (NB, 128), 0)
    padf = (jnp.where(((blk >> 2) == me) & jnp.logical_not(keep), 1.0, 0.0)
            + jnp.where(mine, 1.0, 0.0))
    pcol = jnp.dot(jnp.ones((8, NB), bf16), padf.astype(bf16),
                   preferred_element_type=f32)
    npad = jnp.dot(pcol.astype(bf16), jnp.ones((128, NSLOT), bf16),
                   preferred_element_type=f32)

    s_iota = lax.broadcasted_iota(i32, (NSLOT, 128), 0)
    lane = lax.broadcasted_iota(i32, (1, 128), 1)
    acc = jnp.zeros((NSLOT, 128), i32)
    for b in range(NB):
        m = slot[b:b + 1, :] == s_iota
        acc = acc + jnp.where(m, lane + (b * 128 + 1), 0)
    hilo = jnp.concatenate([(acc >> 6).astype(f32), (acc & 63).astype(f32)],
                           axis=0).astype(bf16)
    red = lax.dot_general(jnp.ones((8, 128), bf16), hilo,
                          (((1,), (1,)), ((), ())),
                          preferred_element_type=f32)
    tok = (red[:, :NSLOT] * 64.0 + red[:, NSLOT:] - 1.0).astype(i32)
    sl = lax.broadcasted_iota(i32, (8, NSLOT), 1)
    sub = lax.broadcasted_iota(i32, (8, NSLOT), 0)
    valid = tok >= 0
    src_row = jnp.where(valid, tok, 0)
    dst_code = jnp.where(valid, ((tok >> 9) << 10) | (tok & (ROWS - 1)),
                         (me << 10) | (ROWS + sl))
    tab = jnp.where(sub == 0, src_row, dst_code)
    tab = jnp.where(sl == SLOT - 1, npad.astype(i32), tab)
    tab_v[...] = tab

    c1 = pltpu.make_async_copy(tab_v.at[pl.ds(0, 1)], tab_s.at[pl.ds(0, 1)],
                               tsem.at[0])
    c2 = pltpu.make_async_copy(tab_v.at[pl.ds(1, 1)], tab_s.at[pl.ds(1, 1)],
                               tsem.at[1])
    c1.start()
    c2.start()
    c1.wait()
    c2.wait()

    gather(0)
    gather(1)

    nd = tab_s[0, SLOT - 1]
    for bit in range(7):
        sz = 8 << bit

        @pl.when(((nd >> (3 + bit)) & 1) == 1)
        def _(sz=sz):
            pltpu.make_async_copy(pad_src.at[pl.ds(0, sz)],
                                  pad_dst.at[pl.ds(sz, sz)], recv_sem).start()
    for j in range(7):
        @pl.when((nd & 7) > j)
        def _(j=j):
            pltpu.make_async_copy(pad_src.at[pl.ds(j, 1)],
                                  pad_dst.at[pl.ds(j, 1)], recv_sem).start()

    pl.semaphore_wait(barrier, NDEV - 1)

    n8 = (CAP // 8) * 8
    for e in range(E_LOC):
        pltpu.make_async_copy(xg.at[e, pl.ds(0, n8)], xg.at[e, pl.ds(0, n8)],
                              gsem.at[e]).wait()
        for s in range(n8, CAP):
            pltpu.make_async_copy(xg.at[e, pl.ds(s, 1)], xg.at[e, pl.ds(s, 1)],
                                  gsem.at[e]).wait()
        if e < last:
            w_copy(e).wait()
            y = jnp.dot(xg[e].astype(bf16), wbuf[e].astype(bf16),
                        preferred_element_type=f32)
            res[e, :, :QW] = pack(y[:, :HW])
            res[e, :, QW:] = pack(y[:, HW:])
            send_rows(e, 0, HW)
        else:
            w_last_copy(0).wait()
            y = jnp.dot(xg[e].astype(bf16), wbuf[e, :, :HW].astype(bf16),
                        preferred_element_type=f32)
            res[e, :, :QW] = pack(y)
            send_rows(e, 0, QW)
            y = None
            for k in range(KSPLIT):
                w_last_copy(k + 1).wait()
                p = jnp.dot(xg[e, :, k * kc:(k + 1) * kc].astype(bf16),
                            wbuf[e, k * kc:(k + 1) * kc, HW:].astype(bf16),
                            preferred_element_type=f32)
                y = p if y is None else y + p
            res[e, :, QW:] = pack(y)
            send_rows(e, QW, QW)
        if e + 2 < E_LOC:
            gather(e + 2)

    pltpu.make_async_remote_copy(
        stage.at[pl.ds(0, NSEND)], stage.at[pl.ds(0, NSEND)],
        send_sem, recv_sem, device_id=(me,),
        device_id_type=pl.DeviceIdType.MESH).wait_send()
    pltpu.make_async_copy(stage.at[pl.ds(0, RECV_ROWS)],
                          stage.at[pl.ds(0, RECV_ROWS)], recv_sem).wait()
    w = stage[pl.ds(0, ROWS), :]
    lo = lax.bitcast_convert_type(w << 16, f32)
    hi = lax.bitcast_convert_type(w & jnp.uint32(0xFFFF0000), f32)
    out_ref[:, 0 * QW:1 * QW] = lo[:, :QW]
    out_ref[:, 1 * QW:2 * QW] = hi[:, :QW]
    out_ref[:, 2 * QW:3 * QW] = lo[:, QW:]
    out_ref[:, 3 * QW:4 * QW] = hi[:, QW:]


def pallas_dist_moe_cap_ep_outshard_n2048_d512_e8_h1024_kernel(
    x: jax.Array,
    router_W: jax.Array,
    route_idx: jax.Array,
    expert_W: jax.Array,
):
    del router_W
    idx2d = route_idx.astype(jnp.int32).reshape(NB, 128)
    return pl.pallas_call(
        _kernel,
        out_shape=jax.ShapeDtypeStruct((ROWS, H), jnp.float32),
        in_specs=[
            pl.BlockSpec(memory_space=pl.ANY),
            pl.BlockSpec(memory_space=pl.ANY),
            pl.BlockSpec(memory_space=pl.ANY),
        ],
        out_specs=pl.BlockSpec(memory_space=pltpu.VMEM),
        scratch_shapes=[
            pltpu.VMEM((NB, 128), jnp.int32),
            pltpu.VMEM((E_LOC, D, H), jnp.float32),
            pltpu.VMEM((E_LOC, MROWS, D), jnp.float32),
            pltpu.VMEM((E_LOC, MROWS, HW), jnp.uint32),
            pltpu.VMEM((2 * ROWS, HW), jnp.uint32),
            pltpu.VMEM((ROWS, HW), jnp.uint32),
            pltpu.VMEM((2 * ROWS, HW), jnp.uint32),
            pltpu.VMEM((8, NSLOT), jnp.int32),
            pltpu.SMEM((2, NSLOT), jnp.int32),
            pltpu.SemaphoreType.DMA,
            pltpu.SemaphoreType.DMA((E_LOC + KSPLIT,)),
            pltpu.SemaphoreType.DMA((E_LOC,)),
            pltpu.SemaphoreType.DMA((2,)),
            pltpu.SemaphoreType.DMA,
            pltpu.SemaphoreType.DMA,
        ],
        compiler_params=pltpu.CompilerParams(
            collective_id=0,
            vmem_limit_bytes=64 * 1024 * 1024,
            disable_bounds_checks=True,
        ),
    )(idx2d, x, expert_W)
```
